```python
import numpy as np

kernel_name = "dist_ag_xy_y_m1024_n512"

def setup_inputs():
    return {"x": np.random.randn(2048, 512).astype(np.float32)}

def reference(x: np.ndarray) -> np.ndarray:
    return x
```

```python
import functools

import jax
import jax.numpy as jnp
from jax import lax
from jax.experimental import pallas as pl
from jax.experimental.pallas import tpu as pltpu

_MESH = pl.DeviceIdType.MESH

_M = 1024
_N = 512
_RB = 16
_CT = _N // 128
_NU = (_M // _RB) * _CT

_U = {(0, 0): 140, (0, 1): 138, (1, 0): 132, (1, 1): 132}
_ND = {(0, 0): 0, (0, 1): 2, (1, 0): 0, (1, 1): 0}
_GN = 4
_GX = 4
_WINDOW = 48
_LAG = {(0, 0): 28, (1, 0): 14, (0, 1): 28, (1, 1): 14}
_LOAD_RBS = (1, 1, 2, 4, 8, 64)


def _split(lo, hi, g):
    out = []
    while lo < hi:
        n = min(g, hi - lo)
        out.append((lo, n))
        lo += n
    return out


def _ychunks(dev):
    fwd = _NU - _U[(1 - dev[0], dev[1])]
    return [(p, n, True) for p, n in _split(0, fwd, 1)] + [
        (p, n, False) for p, n in _split(fwd, _U[dev] - _ND[dev], _GN)
    ]


def _unit(dev, p, n):
    return p if dev[0] == 0 else _NU - p - n


_NY = max(len(_ychunks(d)) for d in _U)
_NX = max(len(_split(0, _NU - _U[d], _GX)) for d in _U)
_NDMAX = max(1, max(_ND.values()))


def _body(
    x_ref,
    out_ref,
    sbuf,
    rbuf,
    load_sems,
    rest_sem,
    ysend,
    yrecv,
    xsend,
    xrecv,
    ack_y,
    ack_x,
    dsend,
    drecv,
):
    mx = lax.axis_index("x")
    my = lax.axis_index("y")
    bar = pltpu.get_barrier_semaphore()

    def signal(sem, dev):
        pl.semaphore_signal(sem, inc=1, device_id=dev, device_id_type=_MESH)

    def wait_bytes(ref, sem):
        pltpu.make_async_copy(ref, ref, sem).wait()

    def dev_body(dx, dy):
        me = (dx, dy)
        ynbr = (dx, 1 - dy)
        xnbr = (1 - dx, dy)
        diag = (1 - dx, 1 - dy)
        mybase = dy * _M
        otbase = (1 - dy) * _M
        n_bf16 = _U[me] - _ND[me]

        def cast_down(u):
            rb, ct = divmod(u, _CT)
            sbuf[u] = out_ref[
                pl.ds(mybase + rb * _RB, _RB), pl.ds(ct * 128, 128)
            ].astype(jnp.bfloat16)

        def cast_up(u):
            rb, ct = divmod(u, _CT)
            out_ref[pl.ds(otbase + rb * _RB, _RB), pl.ds(ct * 128, 128)] = rbuf[
                u
            ].astype(jnp.float32)

        def direct(dev, i):
            u = _unit(dev, _U[dev] - _ND[dev] + i, 1)
            rb, ct = divmod(u, _CT)
            return pltpu.make_async_remote_copy(
                src_ref=x_ref.at[pl.ds(rb * _RB, _RB), pl.ds(ct * 128, 128)],
                dst_ref=out_ref.at[
                    pl.ds(dev[1] * _M + rb * _RB, _RB), pl.ds(ct * 128, 128)
                ],
                send_sem=dsend.at[i],
                recv_sem=drecv.at[i],
                device_id=(dev[0], 1 - dev[1]),
                device_id_type=_MESH,
            )

        if dy == 0:
            signal(bar, ynbr)
        if dx == 0:
            signal(bar, xnbr)

        def handshake():
            pl.semaphore_wait(bar, dx + dy)
            if dy == 1:
                for j in range(_ND[me]):
                    direct(me, j).start()
                signal(ack_y, ynbr)
            if dx == 1:
                signal(ack_x, xnbr)

        nrb_send = -(-n_bf16 // _CT)
        loads = []
        p = 0
        for i, n in enumerate(_LOAD_RBS):
            n = min(n, nrb_send - p)
            if n <= 0:
                break
            r0 = p * _RB if dx == 0 else _M - (p + n) * _RB
            cp = pltpu.make_async_copy(
                x_ref.at[pl.ds(r0, n * _RB)],
                out_ref.at[pl.ds(mybase + r0, n * _RB)],
                load_sems.at[i],
            )
            cp.start()
            p += n
            loads.append((p, cp))
            if i == 0 and dx + dy == 1:
                handshake()
        assert p == nrb_send
        nrest = _M - nrb_send * _RB
        rs = nrb_send * _RB if dx == 0 else 0
        rest = pltpu.make_async_copy(
            x_ref.at[pl.ds(rs, nrest)],
            out_ref.at[pl.ds(mybase + rs, nrest)],
            rest_sem,
        )
        rest.start()
        if dx + dy == 2:
            handshake()

        sch = _ychunks(me)

        def send(k):
            p0, n, _ = sch[k]
            u0 = _unit(me, p0, n)
            pltpu.make_async_remote_copy(
                src_ref=sbuf.at[pl.ds(u0, n)],
                dst_ref=rbuf.at[pl.ds(u0, n)],
                send_sem=ysend,
                recv_sem=yrecv.at[k],
                device_id=ynbr,
                device_id_type=_MESH,
            ).start()

        st = dict(li=0, loaded=0, cast=0)

        def ensure(upto):
            upto = min(upto, n_bf16)
            while st["loaded"] < upto:
                pe, cp = loads[st["li"]]
                cp.wait()
                st["li"] += 1
                st["loaded"] = min(pe * _CT, n_bf16)
            for q in range(st["cast"], upto):
                cast_down(_unit(me, q, 1))
            st["cast"] = max(st["cast"], upto)

        nfirst = min(_WINDOW, len(sch))
        first_end = sch[nfirst - 1][0] + sch[nfirst - 1][1]
        sent = 0
        while sent < nfirst:
            need = sch[sent][0] + sch[sent][1]
            if need > st["cast"]:
                ensure(need)
                ensure(min(st["loaded"], first_end))
            if sent == 0 and dy == 0:
                pl.semaphore_wait(ack_y, 1)
                for j in range(_ND[me]):
                    direct(me, j).start()
            send(sent)
            sent += 1
        if dx == 0:
            pl.semaphore_wait(ack_x, 1)

        rch = _ychunks(ynbr)
        xgroups = _split(0, _NU - _U[ynbr], _GX)

        def take_x(j):
            p0, n = xgroups[j]
            u0 = _unit(diag, p0, n)
            wait_bytes(rbuf.at[pl.ds(u0, n)], xrecv.at[j])
            for u in range(u0, u0 + n):
                cast_up(u)

        xj = 0
        for k, (p0, n, fwd) in enumerate(rch):
            u0 = _unit(ynbr, p0, n)
            wait_bytes(rbuf.at[pl.ds(u0, n)], yrecv.at[k])
            if fwd:
                pltpu.make_async_remote_copy(
                    src_ref=rbuf.at[pl.ds(u0, n)],
                    dst_ref=rbuf.at[pl.ds(u0, n)],
                    send_sem=xsend,
                    recv_sem=xrecv.at[p0 // _GX],
                    device_id=xnbr,
                    device_id_type=_MESH,
                ).start()
            if sent < len(sch):
                ensure(sch[sent][0] + sch[sent][1])
                send(sent)
                sent += 1
            for u in range(u0, u0 + n):
                cast_up(u)
            while (
                xj < len(xgroups)
                and xgroups[xj][0] + xgroups[xj][1] + _LAG[me] <= p0 + n
            ):
                take_x(xj)
                xj += 1
        assert sent == len(sch) and st["li"] == len(loads)
        while xj < len(xgroups):
            take_x(xj)
            xj += 1

        for j in range(_ND[ynbr]):
            direct(ynbr, j).wait_recv()
        for j in range(_ND[me]):
            direct(me, j).wait_send()
        wait_bytes(sbuf.at[pl.ds(_unit(me, 0, n_bf16), n_bf16)], ysend)
        n_fwd = _NU - _U[diag]
        wait_bytes(rbuf.at[pl.ds(_unit(ynbr, 0, n_fwd), n_fwd)], xsend)
        rest.wait()

    for dx in range(2):
        for dy in range(2):
            pl.when(jnp.logical_and(mx == dx, my == dy))(
                functools.partial(dev_body, dx, dy)
            )


def pallas_dist_ag_xy_y_m1024_n512_kernel(
    x: jax.Array,
):
    m, n = x.shape
    assert (m, n) == (_M, _N)
    return pl.pallas_call(
        _body,
        out_shape=jax.ShapeDtypeStruct((2 * m, n), x.dtype),
        in_specs=[pl.BlockSpec(memory_space=pl.ANY)],
        out_specs=pl.BlockSpec(memory_space=pltpu.VMEM),
        scratch_shapes=[
            pltpu.VMEM((_NU, _RB, 128), jnp.bfloat16),
            pltpu.VMEM((_NU, _RB, 128), jnp.bfloat16),
            pltpu.SemaphoreType.DMA((len(_LOAD_RBS),)),
            pltpu.SemaphoreType.DMA,
            pltpu.SemaphoreType.DMA,
            pltpu.SemaphoreType.DMA((_NY,)),
            pltpu.SemaphoreType.DMA,
            pltpu.SemaphoreType.DMA((_NX,)),
            pltpu.SemaphoreType.REGULAR,
            pltpu.SemaphoreType.REGULAR,
            pltpu.SemaphoreType.DMA((_NDMAX,)),
            pltpu.SemaphoreType.DMA((_NDMAX,)),
        ],
        compiler_params=pltpu.CompilerParams(
            collective_id=0, disable_semaphore_checks=True
        ),
    )(x)
```
